```python
import numpy as np

kernel_name = "dist_mlpseq_tp1d_bs_rep_b64_d1024_h2048"

def setup_inputs():
    x = np.random.randn(256, 1024).astype(np.float32)
    Win0 = np.random.randn(1024, 8192).astype(np.float32)
    Wout0 = np.random.randn(8192, 1024).astype(np.float32)
    Win1 = np.random.randn(1024, 8192).astype(np.float32)
    Wout1 = np.random.randn(8192, 1024).astype(np.float32)
    Win2 = np.random.randn(1024, 8192).astype(np.float32)
    Wout2 = np.random.randn(8192, 1024).astype(np.float32)
    return {"x": x, "Win0": Win0, "Wout0": Wout0, "Win1": Win1, "Wout1": Wout1, "Win2": Win2, "Wout2": Wout2}

def reference(x, Win0, Win1, Win2, Wout0, Wout1, Wout2):
    h = x @ Win0
    h = np.maximum(h, 0.0)
    x = h @ Wout0
    h = x @ Win1
    h = np.maximum(h, 0.0)
    x = h @ Wout1
    h = x @ Win2
    h = np.maximum(h, 0.0)
    x = h @ Wout2
    return x
```

```python
import contextlib
import jax
import jax.numpy as jnp
from jax import lax
from jax.experimental import pallas as pl
from jax.experimental.pallas import tpu as pltpu

MESH = pl.DeviceIdType.MESH
BF = jnp.bfloat16
F32 = jnp.float32
B, D, H = 256, 1024, 2048
NU = D // 128
Q = 64


def make(blocks, scheme, sched, nsub=4, stair=None, hw=512, lag2=2, lag3=4, tr=False, odt=BF, msplit=1, flags=None):
    sc = (lambda n: jax.named_scope('@' + n)) if tr else (lambda n: contextlib.nullcontext())
    phys = {u: c0 + i for us, _, c0 in blocks for i, u in enumerate(us)}
    a_units = [u for u in range(NU) if scheme[u] == 'A']
    nsub = {u: (nsub if isinstance(nsub, int) else nsub[u]) for u in a_units}
    qoff = {}
    for u in a_units:
        qoff[u] = sum(nsub[v] for v in a_units if v < u)
    nq2 = max(1, sum(nsub.values()))
    na = max(1, len(a_units))
    b01 = ((0, 3), (5, 3), (3, 2))
    dmas, need, pre = [], {}, {}
    for bi, (us, ks, c0) in enumerate(blocks):
        if stair and bi in stair:
            r, nb = stair[bi]
            cs = [phys[u] for j in range(bi, bi + nb) for u in blocks[j][0]]
            assert sorted(cs) == list(range(min(cs), min(cs) + len(cs)))
            dmas.append((0, r, min(cs), len(cs)))
            need.setdefault((bi, 0), []).append(len(dmas) - 1)
            for j in range(bi, bi + nb):
                pre[j] = r
        off = 0
        for k, r in enumerate(ks):
            r0 = max(off, pre.get(bi, 0))
            if off + r > r0:
                dmas.append((r0, off + r - r0, c0, len(us)))
                need.setdefault((bi, k), []).append(len(dmas) - 1)
            off += r

    def fn(x, a0, b0, a1, b1, a2, b2):
        def body(x_hbm, a0, b0, a1, b1, a2, b2, o_ref,
                 wa, wb, xin, xg, h, ybf, s1r, s2s, s2r, tacc, tbf, t1r, t2s, t2r,
                 wsem, gsem, r1sem, r2sem, r3sem, q1sem, q2sem, ssem):
            def start_a(l):
                for j in range(4):
                    s = (slice(None), pl.ds(j * 512, 512))
                    pltpu.make_async_copy((a0, a1, a2)[l].at[s], wa.at[l].at[s], wsem.at[1 + 7 * l + j]).start()

            def start_b(l):
                for j, (u0, w) in enumerate(b01):
                    s = (slice(None), pl.ds(u0 * 128, w * 128))
                    pltpu.make_async_copy((b0, b1)[l].at[s], wb.at[l].at[s], wsem.at[5 + 7 * l + j]).start()

            def tail_cp(i):
                r0, nr, c0, w = dmas[i]
                s = (pl.ds(r0, nr), pl.ds(c0 * 128, w * 128))
                return pltpu.make_async_copy(b2.at[s], wb.at[2].at[s], wsem.at[19 + i])

            xcp = pltpu.make_async_copy(x_hbm, xin, wsem.at[0])
            xcp.start()
            start_a(0)
            me = lax.axis_index("i")
            p1 = me ^ 1
            p2 = 3 - me
            pd = me ^ 2
            ka = (me ^ (me >> 1)) & 1
            kb = 2 + (me >> 1)

            def rcopy(src, dst, rsem, to):
                return pltpu.make_async_remote_copy(src, dst, ssem, rsem, device_id=(to,), device_id_type=MESH)

            def wait_all(ref, sem):
                pltpu.make_async_copy(ref, ref, sem).wait()

            bar = pltpu.get_barrier_semaphore()
            for p in (pd, p1, p2):
                pl.semaphore_signal(bar, inc=1, device_id=(p,), device_id_type=MESH)
            start_b(0)
            start_a(1)
            xcp.wait()
            for u in range(NU):
                xg[0, me, u] = xin[:, u * 128:(u + 1) * 128].astype(BF)
            pl.semaphore_wait(bar, 3)
            for p in (pd, p1, p2):
                rcopy(xg.at[0, me], xg.at[0, me], gsem, p).start()
            with sc('xg'):
                wait_all(xg.at[0, pl.ds(0, 3)], gsem)

            def step1(l, u):
                rcopy(ybf.at[l, u, 1 - ka], s1r.at[l, u, 0], r1sem.at[u], p1).start()
                rcopy(ybf.at[l, u, 5 - kb], s1r.at[l, u, 1], r1sem.at[u], p2).start()

            def step2(l, u):
                wait_all(s1r.at[l, u], r1sem.at[u])
                s2s[l, u, 0] = (ybf[l, u, ka].astype(F32) + s1r[l, u, 0].astype(F32)).astype(BF)
                s2s[l, u, 1] = (ybf[l, u, kb].astype(F32) + s1r[l, u, 1].astype(F32)).astype(BF)
                rcopy(s2s.at[l, u, 0], s2r.at[l, u, 0], r2sem.at[u], p2).start()
                rcopy(s2s.at[l, u, 1], s2r.at[l, u, 1], r2sem.at[u], p1).start()

            def step3(l, u, dst):
                wait_all(s2r.at[l, u], r2sem.at[u])
                for half, (k, p) in enumerate(((ka, p1), (kb, p2))):
                    d = dst(k)
                    d[...] = (s2s[l, u, half].astype(F32) + s2r[l, u, half].astype(F32)).astype(BF)
                    rcopy(d, d, r3sem, p).start()

            def hphase(l):
                def hstep(j, c):
                    @pl.when(j % (512 // hw) == 0)
                    def _():
                        wait_all(wa.at[l, :, pl.ds(0, 512)], wsem.at[1 + 7 * l + j // (512 // hw)])
                    cols = pl.ds(pl.multiple_of(j * hw, hw), hw)
                    xv = jnp.concatenate([xg[l, :, u].reshape(B, 128) for u in range(NU)], axis=1)
                    acc = jnp.dot(xv, wa[l, :, cols].astype(BF), preferred_element_type=F32)
                    h[:, cols] = jnp.maximum(acc, 0.0).astype(BF)
                    return c
                with sc('h'):
                    lax.fori_loop(0, H // hw, hstep, 0)

            def unit(i):
                return jnp.where(i < 3, i, jnp.where(i < 6, i + 2, i - 3))

            def layer(l, carry):
                @pl.when(l == 2)
                def _():
                    for i in range(len(dmas)):
                        tail_cp(i).start()
                hphase(l)

                @pl.when(l < 2)
                def _():
                    @pl.when(l == 0)
                    def _():
                        start_b(1)
                        start_a(2)

                    def ystep(i, c):
                        @pl.when(i < NU)
                        def _():
                            @pl.when(jnp.logical_or(i == 0, i == 3))
                            def _():
                                wait_all(wb.at[l, :, pl.ds(0, 384)], wsem.at[5 + 7 * l + i // 3])

                            @pl.when(i == 6)
                            def _():
                                wait_all(wb.at[l, :, pl.ds(0, 256)], wsem.at[7 + 7 * l])
                            u = unit(i)
                            cols = pl.ds(pl.multiple_of(u * 128, 128), 128)
                            y = jnp.dot(h[...], wb[l, :, cols].astype(BF), preferred_element_type=F32)
                            ybf[l, u] = y.astype(BF).reshape(4, Q, 128)
                            step1(l, u)

                        @pl.when(jnp.logical_and(i >= lag2, i < NU + lag2))
                        def _():
                            step2(l, unit(i - lag2))

                        @pl.when(i >= lag3)
                        def _():
                            u = unit(i - lag3)
                            step3(l, u, lambda k: xg.at[l + 1, k, u])
                        return c

                    with sc('y'):
                        lax.fori_loop(0, NU + lag3, ystep, 0)
                    with sc('xw'):
                        wait_all(xg.at[l + 1, pl.ds(0, 2)], r3sem)
                return carry

            lax.fori_loop(0, 3, layer, 0)

            def mm(bi, k):
                us, ks, c0 = blocks[bi]
                for i in need.get((bi, k), []):
                    tail_cp(i).wait()
                w = len(us) * 128
                rows = pl.ds(sum(ks[:k]), ks[k])
                final = k == len(ks) - 1
                wv = wb[2, rows, pl.ds(c0 * 128, w)].astype(BF)
                if final and scheme[us[0]] == 'A' and len(us) == 1:
                    u = us[0]
                    ai, ns = a_units.index(u), nsub[u]
                    sub = 128 // ns
                    groups = [list(range(ns))] if msplit == 1 else [list(range(ns))[g * ns // msplit:(g + 1) * ns // msplit] for g in range(msplit)]
                    for g in groups:
                        rs = pl.ds(g[0] * 2 * sub, len(g) * 2 * sub)
                        y = jnp.dot(h[rs, rows], wv, preferred_element_type=F32)
                        if k > 0:
                            y = y + tacc[rs, :w]
                        tbf[ai, rs] = y.astype(BF)
                        for i in g:
                            for half, p in ((0, p1), (1, p2)):
                                r = pl.ds((2 * i + half) * sub, sub)
                                rcopy(tbf.at[ai, r], t1r.at[ai, r], q1sem.at[qoff[u] + i], p).start()
                    return
                y = jnp.dot(h[:, rows], wv, preferred_element_type=F32)
                if k > 0:
                    y = y + tacc[:, :w]
                if not final:
                    tacc[:, :w] = y
                    return
                for j, u in enumerate(us):
                    assert scheme[u] == 'C'
                    ybf[2, u] = y[:, j * 128:(j + 1) * 128].astype(BF).reshape(4, Q, 128)
                    step1(2, u)

            def ocols(u):
                return pl.ds(phys[u] * 128, 128)

            def a2(u, i):
                ai, sub = a_units.index(u), 128 // nsub[u]
                r2 = pl.ds(2 * i * sub, 2 * sub)
                wait_all(t1r.at[ai, r2], q1sem.at[qoff[u] + i])
                t2s[ai, r2] = (tbf[ai, r2].astype(F32) + t1r[ai, r2].astype(F32)).astype(BF)
                for half, p in ((0, p2), (1, p1)):
                    r = pl.ds((2 * i + half) * sub, sub)
                    rcopy(t2s.at[ai, r], t2r.at[ai, r], q2sem.at[qoff[u] + i], p).start()

            def a3(u, i):
                ai, sub = a_units.index(u), 128 // nsub[u]
                r2 = pl.ds(2 * i * sub, 2 * sub)
                wait_all(t2r.at[ai, r2], q2sem.at[qoff[u] + i])
                o_ref[r2, ocols(u)] = (t2s[ai, r2].astype(F32) + t2r[ai, r2].astype(F32)).astype(BF)

            def finish_c():
                wait_all(xg.at[0, pl.ds(0, 2), pl.ds(0, NU - len(a_units))], r3sem)

            for op in sched:
                with sc(''.join(map(str, op))):
                    if op[0] == 'mm':
                        mm(op[1], op[2])
                    elif op[0] == 's2':
                        step2(2, op[1])
                    elif op[0] == 's3':
                        step3(2, op[1], lambda k: o_ref.at[pl.ds(pl.multiple_of(k * Q, Q), Q), ocols(op[1])])
                    elif op[0] == 'a2':
                        a2(op[1], op[2])
                    elif op[0] == 'a3':
                        a3(op[1], op[2])
                    elif op[0] == 'w':
                        finish_c()
            nq = 3 * NU + 6 * (3 * NU - len(a_units)) + 8 * len(a_units)
            wait_all(wb.at[0, pl.ds(0, nq * 8), pl.ds(0, 512)], ssem)

        DMA = pltpu.SemaphoreType.DMA
        out = pl.pallas_call(
            body,
            out_shape=jax.ShapeDtypeStruct((B, D), BF),
            in_specs=[pl.BlockSpec(memory_space=pltpu.HBM)] * 7,
            out_specs=pl.BlockSpec(memory_space=pltpu.VMEM),
            scratch_shapes=[
                pltpu.VMEM((3, D, H), F32), pltpu.VMEM((3, H, D), F32),
                pltpu.VMEM((Q, D), F32), pltpu.VMEM((3, 4, NU, Q, 128), BF), pltpu.VMEM((B, H), BF),
                pltpu.VMEM((3, NU, 4, Q, 128), BF),
                pltpu.VMEM((3, NU, 2, Q, 128), BF), pltpu.VMEM((3, NU, 2, Q, 128), BF), pltpu.VMEM((3, NU, 2, Q, 128), BF),
                pltpu.VMEM((B, 384), F32),
                pltpu.VMEM((na, B, 128), BF), pltpu.VMEM((na, B, 128), BF), pltpu.VMEM((na, B, 128), BF), pltpu.VMEM((na, B, 128), BF),
                DMA((19 + len(dmas),)), DMA, DMA((NU,)), DMA((NU,)), DMA, DMA((nq2,)), DMA((nq2,)), DMA,
            ],
            compiler_params=pltpu.CompilerParams(
                vmem_limit_bytes=100 * 2**20, collective_id=0, flags=flags,
                disable_semaphore_checks=True, disable_bounds_checks=True),
        )(x, a0, b0, a1, b1, a2, b2)
        return out.astype(odt)

    return fn


def parse(s):
    return [(t[:2], *map(int, t[2:])) if len(t) > 1 else (t,) for t in s.split()]


k1, k2, ks = [2048], [1024, 1024], [1536, 512]
B221111 = [((0, 1), k2, 1), ((2, 3), k2, 3), ((4,), ks, 5), ((5,), ks, 6), ((6,), ks, 7), ((7,), ks, 0)]
SA = parse("mm00 mm01 mm10 s20 s21 mm11 s30 mm20 mm21 s22 s23 s31 mm30 s24 mm31 s32 mm40 s33 mm41 s25 s34 mm50 mm51 "
           "a260 a261 a262 a263 s35 a270 a271 a272 a273 a360 a361 a362 a363 a370 a371 w a372 a373")


def pallas_dist_mlpseq_tp1d_bs_rep_b64_d1024_h2048_kernel(x, Win0, Wout0, Win1, Wout1, Win2, Wout2):
    return make(B221111, 'CCCCCCAA', SA, msplit=4)(x, Win0, Wout0, Win1, Wout1, Win2, Wout2)
```

```python
import jax
import jax.numpy as jnp
from jax import lax
from jax.experimental import pallas as pl
from jax.experimental.pallas import tpu as pltpu

BF16 = jnp.bfloat16
F32 = jnp.float32

LAYERS = 3
B, D, H = 256, 1024, 2048
Q = B // 4
LANES = 128
UNITS = D // LANES
WIDE, N_WIDE, NARROW, N_NARROW = 512, 3, 256, 2
H_BLOCKS = N_WIDE + N_NARROW
TRADED = 128
TRADE_AFTER = (range(1, 6), range(6, 8))

K_CHUNKS = (2, 2, 2, 2, 4, 4, 4, 4)
QUEUE_AFTER = {4: (1, 0), 5: (2, 0), 6: (3, 0), 7: (4, 0)}
PIECES = (
    "PQ", "PQ", "PQ", "PQ", "PPQQ", "PPQQ", "PPPAQQQQ", "AAAAAAAA",
)
SCHEDULE = (
    """
    mm00 mm01 a101 mm10 mm11 a111 mm20 b100 mm21 a121 mm30 b110 mm31 a131 b200 mm40 mm41
    b120 mm42 mm43 a142 a143 b210 mm50 mm51 mm52 b130 mm53 a153 a152 mm60 mm61 b140 mm62
    b141 mm63 a166 a165 a167 b220 a164 mm70 mm71 b151 mm72 b150 mm73 b163 b162 b160 b161
    b240 b230 b241 b170 b171 b172 b173 b174 b175 b176 b177 b251 b250 b260 f063 b262 b261
    ow90 f071 f070 f072 f073 f074 f076 f075 f077
    """,
    """
    mm00 mm01 m101 m100 mm10 mm11 m111 m110 mm20 m200 m201 mm21 m121 m120 mm30 m211 m210
    mm31 m131 m130 m301 mm40 m221 m300 mm41 m311 mm42 mm43 m140 m142 m143 m141 m220 m231
    m310 mm50 mm51 m321 mm52 m242 m230 mm53 m153 m151 m152 m150 mm60 mm61 m331 mm62 m240
    m243 mm63 m162 m160 m167 m161 m165 m166 m164 m241 mm70 m342 m343 mm71 m250 mm72 m251
    mm73 m266 m267 n263 m265 m252 m264 m253 m263 m260 n270 m262 m352 n271 m261 m353 n272
    n274 n273 n276 n275 n277 m330 m367 m320 m350 m340 m365 m341 m362 fn63 m351 m366 m361
    m364 m360 m270 m271 m272 m273 m274 m275 m276 m277 fn70 ff63 ff70 fn72 fn71 ff72 fn73
    ff71 fn74 ff73 ff75 fn75 fn76 ff74 fn77 ff76 ff77 ow90
    """,
    """
    mm00 mm01 a100 mm10 mm11 a110 b101 mm20 b111 mm21 a120 b201 mm30 b121 mm31 a130 mm40
    b211 mm41 mm42 b131 mm43 a140 b221 a141 mm50 mm51 b142 mm52 b143 mm53 a150 a151 b231
    mm60 mm61 b153 mm62 b152 mm63 a160 a162 a161 mm70 mm71 b167 b165 mm72 b166 b164 mm73
    e263 e270 e272 e271 e273 e275 e274 e276 e277 b242 b266 b243 b267 f263 b265 b252 b264
    b253 f270 f272 f271 f273 f274 f276 f277 f275 ow90
    """,
)


def _build(k_chunks, pieces, schedule, queue_after):
    pieces = [[(c, B // 2 // len(p)) for c in p] for p in pieces]
    slots = []
    for steps in schedule:
        chunks, between = [], []
        for step in steps.split():
            step = (step[:2], int(step[2]), int(step[3]))
            if step[0] == "mm":
                chunks.append(step[1:])
                between.append([])
            else:
                between[-1].append(step)
        slots.append(between)
    piece_sem = {}
    for u in range(UNITS):
        for i in range(len(pieces[u])):
            piece_sem[u, i] = 5 * len(piece_sem)

    def win_sem(l, j):
        return 1 + (H_BLOCKS + UNITS) * l + j

    def wout_sem(l, j):
        return win_sem(l, H_BLOCKS + j)

    def body(x_hbm, win0, wout0, win1, wout1, win2, wout2, out_ref,
             win, wout, x_f32, act, h, y, rs_in, half_sum, half_in, acc, own, part, inbox,
             w_sems, x_send, x_recv, ar_send, rs_recv, half_recv, ag_recv, last_send, last_recv,
             trade_send, trade_recv):

        def wait_filled(ref, sem):
            pltpu.make_async_copy(ref, ref, sem).wait()

        def start_win(l):
            for c in range(TRADED if l == LAYERS - 1 else 0, H, LANES):
                j = c // WIDE if c < N_WIDE * WIDE else N_WIDE + (c - N_WIDE * WIDE) // NARROW
                cols = pl.ds(c, LANES)
                pltpu.make_async_copy((win0, win1, win2)[l].at[:, cols], win.at[l, :, cols],
                                      w_sems.at[win_sem(l, j)]).start()

        def start_wout(l, u, groups, sem):
            cols = pl.ds(u * LANES, LANES)
            for e in range(2):
                tile = pl.ds(8 * e, 8)
                pltpu.make_async_copy((wout0, wout1, wout2)[l].at[groups, tile, cols],
                                      wout.at[l, u, groups, tile], w_sems.at[sem]).start()

        all_groups = pl.ds(0, H // 16)
        traded_groups = pl.ds(0, TRADED // 16)

        def chunk_groups(u, k, local_only=False):
            n = H // 16 // k_chunks[u]
            skip = TRADED // 16 if local_only and k == 0 else 0
            return pl.ds(k * n + skip, n - skip)

        def start_last_unit(u):
            for k in range(k_chunks[u]):
                start_wout(2, u, chunk_groups(u, k, True), wout_sem(2, chunks.index((u, k))))

        def remote(src, dst, send_sem, recv_sem, to):
            return pltpu.make_async_remote_copy(src, dst, send_sem, recv_sem, device_id=(to,),
                                                device_id_type=pl.DeviceIdType.MESH)

        def add(a, b):
            return (a.astype(F32) + b.astype(F32)).astype(BF16)

        load_x = pltpu.make_async_copy(x_hbm, x_f32, w_sems.at[0])
        load_x.start()
        start_win(0)

        me = lax.axis_index("i")
        nbr1, nbr2, diag = me ^ 1, 3 - me, me ^ 2
        barrier = pltpu.get_barrier_semaphore()
        for peer in (diag, nbr1, nbr2):
            pl.semaphore_signal(barrier, inc=1, device_id=(peer,), device_id_type=pl.DeviceIdType.MESH)

        def trade_win():
            cols = pl.ds(0, TRADED)
            return remote(win2.at[:, cols], win.at[2, :, cols], trade_send, trade_recv.at[UNITS], nbr1)

        def trade_wout(u):
            return remote(wout2.at[traded_groups, :, pl.ds(u * LANES, LANES)], wout.at[2, u, traded_groups],
                          trade_send, trade_recv.at[u], nbr1)

        load_x.wait()
        for u in range(UNITS):
            act[0, me, u] = x_f32[:, u * LANES:(u + 1) * LANES].astype(BF16)
        pl.semaphore_wait(barrier, 3)
        gathers = [remote(act.at[0, me], act.at[0, me], x_send.at[j], x_recv.at[j], peer)
                   for j, peer in enumerate((diag, nbr1, nbr2))]
        for c in gathers:
            c.start()
        trade_win().start()
        trade_wout(0).start()
        for j, peer in enumerate((diag, nbr1, nbr2)):
            wait_filled(act.at[0, peer], x_recv.at[j])
        for c in gathers:
            c.wait_send()

        keep = ((me ^ (me >> 1)) & 1, 2 + (me >> 1))
        give = (1 - keep[0], 5 - keep[1])

        def scatter(l, u):
            for s, to in enumerate((nbr1, nbr2)):
                remote(y.at[l, give[s], u], rs_in.at[l, u, s], ar_send.at[l, s], rs_recv.at[l, u], to).start()

        def exchange(l, u):
            wait_filled(rs_in.at[l, u], rs_recv.at[l, u])
            for s, to in enumerate((nbr2, nbr1)):
                half_sum[l, u, s] = add(y[l, keep[s], u], rs_in[l, u, s])
                remote(half_sum.at[l, u, s], half_in.at[l, u, s], ar_send.at[l, 2], half_recv.at[l, u], to).start()

        def gather(l, u):
            wait_filled(half_in.at[l, u], half_recv.at[l, u])
            for s, to in enumerate((nbr1, nbr2)):
                dst = act.at[l + 1, keep[s], u]
                dst[...] = add(half_sum[l, u, s], half_in[l, u, s])
                remote(dst, dst, ar_send.at[l, 3 + s], ag_recv.at[l, s], to).start()

        def layer(l):
            def hidden(cols):
                xv = jnp.concatenate([act[l, :, u].reshape(B, LANES) for u in range(UNITS)], axis=1)
                pre = jnp.dot(xv, win[l, :, cols].astype(BF16), preferred_element_type=F32)
                h[:, cols] = jnp.maximum(pre, 0.0).astype(BF16)

            @pl.loop(0, N_WIDE)
            def _(j):
                for m in range(LAYERS):
                    for half in range(2):
                        @pl.when(jnp.logical_and(l == m, j == half))
                        def _():
                            for u in range(UNITS // 2 * half, UNITS // 2 * (half + 1)):
                                if m < LAYERS - 1:
                                    start_wout(m, u, all_groups, wout_sem(m, u))
                                elif u not in queue_after:
                                    start_last_unit(u)

                cols = pl.ds(pl.multiple_of(j * WIDE, WIDE), WIDE)
                traded = jnp.logical_and(l == LAYERS - 1, j == 0)

                @pl.when(traded)
                def _():
                    wait_filled(win.at[2, :, pl.ds(TRADED, WIDE - TRADED)], w_sems.at[win_sem(2, 0)])
                    trade_win().wait_recv()

                @pl.when(jnp.logical_not(traded))
                def _():
                    wait_filled(win.at[l, :, cols], w_sems.at[win_sem(l, j)])

                hidden(cols)

            @pl.loop(0, N_NARROW)
            def _(j):
                cols = pl.ds(pl.multiple_of(N_WIDE * WIDE + j * NARROW, NARROW), NARROW)
                wait_filled(win.at[l, :, cols], w_sems.at[win_sem(l, N_WIDE + j)])
                hidden(cols)

            @pl.when(l < LAYERS - 1)
            def _():
                @pl.loop(0, UNITS + 3)
                def _(u):
                    @pl.when(u < UNITS)
                    def _():
                        wait_filled(wout.at[l, u], w_sems.at[wout_sem(l, u)])
                        for m in range(LAYERS - 1):
                            pl.when(jnp.logical_and(l == m, u == 2))(lambda: start_win(m + 1))
                        w = wout[l, u].reshape(H, LANES).astype(BF16)
                        partial = jnp.dot(h[...], w, preferred_element_type=F32)
                        y[l, :, u] = partial.astype(BF16).reshape(4, Q, LANES)
                        scatter(l, u)

                    pl.when(u >= 3)(lambda: gather(l, u - 3))
                    pl.when(jnp.logical_and(u >= 1, u < UNITS + 1))(lambda: exchange(l, u - 1))

                for m in range(LAYERS - 1):
                    @pl.when(l == m)
                    def _():
                        for u in TRADE_AFTER[m]:
                            trade_wout(u).start()

                for s in range(2):
                    wait_filled(y.at[l, give[s]], ar_send.at[l, s])
                wait_filled(half_sum.at[l], ar_send.at[l, 2])
                for s in range(2):
                    wait_filled(act.at[l + 1, keep[s]], ar_send.at[l, 3 + s])
                    wait_filled(act.at[l + 1, give[s]], ag_recv.at[l, s])

        pl.loop(0, LAYERS)(layer)

        near = me >> 1
        far = 1 - near

        def rows(u, i, half=None):
            n = pieces[u][i][1]
            if half is None:
                return pl.ds(2 * n * i, 2 * n)
            start = n * (2 * i + half)
            return pl.ds(start if isinstance(half, int) else pl.multiple_of(start, n), n)

        def out(u, r):
            return out_ref.at[r, pl.ds(u * LANES, LANES)]

        def sem(u, i, j):
            return last_recv.at[piece_sem[u, i] + j]

        views = {"own": lambda u, r: own.at[u, r], "part": lambda u, r: part.at[u, r], "out": out}

        def send(sent, src, u, i, half, j, to):
            r = rows(u, i, half)
            dst = out(u, r) if src == "out" else inbox.at[0 if src == "own" else 1, u, r]
            remote(views[src](u, r), dst, last_send, sem(u, i, j), to).start()
            sent.append((src, u, i, half))

        def wait_sent(sent):
            while sent:
                src, u, i, half = sent.pop(0)
                ref = views[src](u, rows(u, i, half))
                remote(ref, ref, last_send, sem(u, i, 0), me).wait_send()

        def matmul(u, k, sent):
            n = H // k_chunks[u]
            wait_filled(wout.at[2, u, chunk_groups(u, k, True)], w_sems.at[wout_sem(2, chunks.index((u, k)))])
            if k == 0:
                trade_wout(u).wait_recv()
            w = wout[2, u, chunk_groups(u, k)].reshape(n, LANES).astype(BF16)
            partial = jnp.dot(h[:, pl.ds(k * n, n)], w, preferred_element_type=F32)
            if k > 0:
                partial = partial + acc[...]
            if k < k_chunks[u] - 1:
                acc[...] = partial
                return
            for i, (scheme, m) in enumerate(pieces[u]):
                own[u, rows(u, i)] = partial[2 * m * i:2 * m * (i + 1)].astype(BF16)
                if scheme == "A":
                    for half, to in enumerate((nbr2, nbr1)):
                        send(sent, "own", u, i, half, half, to)

        def run(role, name, u, i, sent):
            if name == "ow":
                for v in range(UNITS):
                    for p, (scheme, _) in enumerate(pieces[v]):
                        if scheme != "A" and role == 1:
                            wait_filled(out(v, rows(v, p, far)), sem(v, p, 4))
                        elif (scheme, role) in (("P", 2), ("Q", 0)):
                            wait_filled(out(v, rows(v, p)), sem(v, p, 4))
                wait_sent(sent)
                return
            scheme = pieces[u][i][0]
            if scheme == "A":
                half = {"m2": near, "fn": near, "n2": far, "ff": far}.get(name)
                halves = (0, 1) if half is None else (half,)
                r = rows(u, i, half)
                hop = 1 if name[0] == "f" else 0
                for s in halves:
                    wait_filled(inbox.at[hop, u, rows(u, i, s)], sem(u, i, 2 * hop + s))
                if hop == 1:
                    out(u, r)[...] = add(part[u, r], inbox[1, u, r])
                    return
                part[u, r] = add(own[u, r], inbox[0, u, r])
                for s in halves:
                    to = (nbr1, nbr2)[s] if half is None else (0 if name == "m2" else 2)
                    send(sent, "part", u, i, s, 2 + s, to)
                return
            first, last = (2, 0) if scheme == "P" else (0, 2)
            both, mine = rows(u, i), rows(u, i, near) if role == 1 else None
            if name == "a1":
                for s, to in enumerate((1, 3)):
                    send(sent, "own", u, i, s, 0, to)
            elif name == "m1":
                send(sent, "own", u, i, far, 1, last)
            elif name == "b1":
                wait_filled(inbox.at[0, u, both], sem(u, i, 1))
                part[u, both] = add(own[u, both], inbox[0, u, both])
                for s, to in enumerate((1, 3)):
                    send(sent, "part", u, i, s, 3, to)
            elif name == "m2":
                wait_filled(inbox.at[0, u, mine], sem(u, i, 0))
                part[u, mine] = add(own[u, mine], inbox[0, u, mine])
                send(sent, "part", u, i, near, 2, last)
            elif name == "m3":
                wait_filled(inbox.at[1, u, mine], sem(u, i, 3))
                out(u, mine)[...] = add(part[u, mine], inbox[1, u, mine])
                send(sent, "out", u, i, near, 4, first)
            elif name == "b2":
                wait_filled(inbox.at[1, u, both], sem(u, i, 2))
                out(u, both)[...] = add(part[u, both], inbox[1, u, both])
                for s, to in enumerate((3, 1)):
                    send(sent, "out", u, i, s, 4, to)

        is_role = (me == 0, (me & 1) == 1, me == 2)
        sent = ([], [], [])
        for j, (u, k) in enumerate(chunks):
            shared = []
            matmul(u, k, shared)
            for v, after in queue_after.items():
                if after == (u, k):
                    start_last_unit(v)
            if (u, k) == (2, 0):
                trade_win().wait_send()
                for v in range(UNITS):
                    trade_wout(v).wait_send()
            for role in (2, 1, 0):
                sent[role].extend(shared)
                if slots[role][j]:
                    @pl.when(is_role[role])
                    def _():
                        for step in slots[role][j]:
                            run(role, *step, sent[role])
                        if j == len(chunks) - 1:
                            wait_sent(sent[role])

    dma = pltpu.SemaphoreType.DMA
    return pl.pallas_call(
        body,
        out_shape=jax.ShapeDtypeStruct((B, D), BF16),
        in_specs=[pl.BlockSpec(memory_space=pltpu.HBM)] * 7,
        out_specs=pl.BlockSpec(memory_space=pltpu.VMEM),
        scratch_shapes=[
            pltpu.VMEM((LAYERS, D, H), F32),
            pltpu.VMEM((LAYERS, UNITS, H // 16, 16, LANES), F32),
            pltpu.VMEM((Q, D), F32),
            pltpu.VMEM((LAYERS, 4, UNITS, Q, LANES), BF16),
            pltpu.VMEM((B, H), BF16),
            pltpu.VMEM((LAYERS - 1, 4, UNITS, Q, LANES), BF16),
            pltpu.VMEM((LAYERS - 1, UNITS, 2, Q, LANES), BF16),
            pltpu.VMEM((LAYERS - 1, UNITS, 2, Q, LANES), BF16),
            pltpu.VMEM((LAYERS - 1, UNITS, 2, Q, LANES), BF16),
            pltpu.VMEM((B, LANES), F32),
            pltpu.VMEM((UNITS, B, LANES), BF16),
            pltpu.VMEM((UNITS, B, LANES), BF16),
            pltpu.VMEM((2, UNITS, B, LANES), BF16),
            dma((wout_sem(2, len(chunks)),)),
            dma((3,)), dma((3,)),
            dma((LAYERS - 1, 5)), dma((LAYERS - 1, UNITS)), dma((LAYERS - 1, UNITS)), dma((LAYERS - 1, 2)),
            dma, dma((5 * len(piece_sem),)),
            dma, dma((UNITS + 1,)),
        ],
        compiler_params=pltpu.CompilerParams(
            vmem_limit_bytes=80 * 2**20,
            collective_id=0,
            disable_bounds_checks=True,
            disable_semaphore_checks=True,
        ),
    )


def pallas_dist_mlpseq_tp1d_bs_rep_b64_d1024_h2048_kernel(
    x: jax.Array,
    Win0: jax.Array,
    Wout0: jax.Array,
    Win1: jax.Array,
    Wout1: jax.Array,
    Win2: jax.Array,
    Wout2: jax.Array,
):
    def tiles(w):
        return w.reshape(H // 16, 16, D)

    call = _build(K_CHUNKS, PIECES, SCHEDULE, QUEUE_AFTER)
    return call(x, Win0, tiles(Wout0), Win1, tiles(Wout1), Win2, tiles(Wout2))
```
